```python
import numpy as np

kernel_name = "dist_layernorm_xy_m512_n256"

def setup_inputs():
    x = np.random.randn(1024, 512).astype(np.float32)
    gamma = np.random.randn(512).astype(np.float32)
    beta = np.random.randn(512).astype(np.float32)
    return {"x": x, "gamma": gamma, "beta": beta}

def reference(x: np.ndarray, gamma: np.ndarray, beta: np.ndarray) -> np.ndarray:
    eps = 1e-5
    mean = np.mean(x, axis=1, keepdims=True)
    var = np.var(x, axis=1, keepdims=True)
    return gamma * (x - mean) / np.sqrt(var + eps) + beta
```

```python
import jax
import jax.numpy as jnp
from jax import lax
from jax.experimental import pallas as pl
from jax.experimental.pallas import tpu as pltpu

EPS = 1e-5
LANES = 128
CHUNKS = (128, 128, 128, 128)
SAFE_RATIO = 64.0


def pallas_dist_layernorm_xy_m512_n256_kernel(
    x: jax.Array,
    gamma: jax.Array,
    beta: jax.Array,
):
    m, n = x.shape
    nch = len(CHUNKS)
    offs = [sum(CHUNKS[:i]) for i in range(nch)]
    nblk = m // LANES

    def body(x_hbm, g_hbm, b_hbm, o_ref, xbuf, gbuf, bbuf, sbuf, rbuf, sfix,
             rfix, lsem, gsem, ssem, rsem, fsem):
        def load(i):
            rows = pl.ds(offs[i], CHUNKS[i])
            return pltpu.make_async_copy(x_hbm.at[rows], xbuf.at[rows], lsem.at[i])

        for i in range(nch):
            load(i).start()
        g_copy = pltpu.make_async_copy(g_hbm, gbuf, gsem.at[0])
        b_copy = pltpu.make_async_copy(b_hbm, bbuf, gsem.at[1])
        g_copy.start()
        b_copy.start()

        peer = (lax.axis_index("x"), 1 - lax.axis_index("y"))
        barrier = pltpu.get_barrier_semaphore()
        pl.semaphore_signal(barrier, inc=1, device_id=peer,
                            device_id_type=pl.DeviceIdType.MESH)

        def exchange(i):
            return pltpu.make_async_remote_copy(
                src_ref=sbuf.at[i], dst_ref=rbuf.at[i],
                send_sem=ssem.at[i], recv_sem=rsem.at[i],
                device_id=peer, device_id_type=pl.DeviceIdType.MESH)

        def diag(rows):
            return (lax.broadcasted_iota(jnp.int32, (rows, LANES), 0)
                    == lax.broadcasted_iota(jnp.int32, (rows, LANES), 1))

        def pack(col):
            return jnp.sum(jnp.where(diag(col.shape[0]), col, 0.0), axis=0, keepdims=True)

        def unpack(vec, rows):
            return jnp.sum(jnp.where(diag(rows), vec, 0.0), axis=1, keepdims=True)

        def combine(hm_l, hv_l, hm_r, hv_r):
            delta = hm_r - hm_l
            var = (hv_l + hv_r) + (delta * delta + EPS)
            return hm_r + hm_l, lax.rsqrt(var)

        def normalize(r0, rows, mean, rstd):
            xv = xbuf[pl.ds(r0, rows), :]
            o_ref[pl.ds(r0, rows), :] = (
                (xv - unpack(mean, rows)) * unpack(rstd, rows) * gbuf[...] + bbuf[...])

        for i in range(nch):
            load(i).wait()
            xv = xbuf[pl.ds(offs[i], CHUNKS[i]), :]
            s1 = pack(jnp.sum(xv, axis=1, keepdims=True))
            s2 = pack(jnp.sum(xv * xv, axis=1, keepdims=True))
            hm = s1 * (0.5 / n)
            sbuf[i, 0:1, :] = hm
            sbuf[i, 1:2, :] = s2 * (0.5 / n) - 2.0 * hm * hm
            if i == 0:
                pl.semaphore_wait(barrier, 1)
            exchange(i).start()
        g_copy.wait()
        b_copy.wait()

        bad = jnp.zeros((1, LANES), jnp.float32)
        for i in range(nch):
            if i == nch - 1:
                for j in range(nch):
                    exchange(j).wait_send()
            exchange(i).wait_recv()
            hm_l, hv_l = sbuf[i, 0:1, :], sbuf[i, 1:2, :]
            hm_r, hv_r = rbuf[i, 0:1, :], rbuf[i, 1:2, :]
            ok = ((hm_l * hm_l <= (0.5 * SAFE_RATIO) * hv_l)
                  & (hm_r * hm_r <= (0.5 * SAFE_RATIO) * hv_r))
            bad = jnp.where(ok, bad, 1.0)
            if i == nch - 1:
                redo = jnp.max(bad) > 0.0
            normalize(offs[i], CHUNKS[i], *combine(hm_l, hv_l, hm_r, hv_r))

        @pl.when(redo)
        def _():
            def centered_stats(j, carry):
                xv = xbuf[pl.ds(pl.multiple_of(j * LANES, LANES), LANES), :]
                mu = jnp.sum(xv, axis=1, keepdims=True) * (1.0 / n)
                d = xv - mu
                m2 = jnp.sum(d * d, axis=1, keepdims=True)
                sfix[j, 0:1, :] = pack(mu * 0.5)
                sfix[j, 1:2, :] = pack(m2 * (0.5 / n))
                return carry

            lax.fori_loop(0, nblk, centered_stats, 0)
            fix = pltpu.make_async_remote_copy(
                src_ref=sfix, dst_ref=rfix, send_sem=fsem.at[0], recv_sem=fsem.at[1],
                device_id=peer, device_id_type=pl.DeviceIdType.MESH)
            fix.start()
            fix.wait()

            def renormalize(j, carry):
                normalize(pl.multiple_of(j * LANES, LANES), LANES,
                          *combine(sfix[j, 0:1, :], sfix[j, 1:2, :],
                                   rfix[j, 0:1, :], rfix[j, 1:2, :]))
                return carry

            lax.fori_loop(0, nblk, renormalize, 0)

    any_spec = pl.BlockSpec(memory_space=pl.ANY)
    return pl.pallas_call(
        body,
        out_shape=jax.ShapeDtypeStruct((m, n), x.dtype),
        in_specs=[any_spec, any_spec, any_spec],
        out_specs=pl.BlockSpec(memory_space=pltpu.VMEM),
        scratch_shapes=[
            pltpu.VMEM((m, n), jnp.float32),
            pltpu.VMEM((1, n), jnp.float32),
            pltpu.VMEM((1, n), jnp.float32),
            pltpu.VMEM((nch, 2, LANES), jnp.float32),
            pltpu.VMEM((nch, 2, LANES), jnp.float32),
            pltpu.VMEM((nblk, 2, LANES), jnp.float32),
            pltpu.VMEM((nblk, 2, LANES), jnp.float32),
            pltpu.SemaphoreType.DMA((nch,)),
            pltpu.SemaphoreType.DMA((2,)),
            pltpu.SemaphoreType.DMA((nch,)),
            pltpu.SemaphoreType.DMA((nch,)),
            pltpu.SemaphoreType.DMA((2,)),
        ],
        compiler_params=pltpu.CompilerParams(
            collective_id=0,
            disable_semaphore_checks=True,
            disable_bounds_checks=True,
        ),
    )(x, gamma.reshape(1, n), beta.reshape(1, n))
```

```python
import jax
import jax.numpy as jnp
from jax import lax
from jax.experimental import pallas as pl
from jax.experimental.pallas import tpu as pltpu

EPS = 1e-5
LANES = 128
SUBLANES = 8
CHUNKS = (112, 112, 112, 96, 80)
MXU_ROWS = (0, 64, 64, 56, 48)
SAFE_RATIO = 4.0
MAX_SQUARE = 1e38
HIGH_HALF = -0x10000
SIGN_BIT = -0x80000000
LN2 = 0.6931471805599453


def pallas_dist_layernorm_xy_m512_n256_kernel(
    x: jax.Array,
    gamma: jax.Array,
    beta: jax.Array,
):
    m, n = x.shape
    assert sum(CHUNKS) == m and max(CHUNKS) <= LANES and n == 2 * LANES
    nch = len(CHUNKS)
    offs = [sum(CHUNKS[:i]) for i in range(nch)]
    nblk = m // LANES
    half_inv_n = 0.5 / n

    def body(x_hbm, g_hbm, b_hbm, o_ref, xbuf, gbuf, bbuf, sfix, rfix, hcol,
             vcol, sbuf, rbuf, lsem, gsem, ssem, rsem, fsem):
        def load(i):
            rows = pl.ds(offs[i], CHUNKS[i])
            return pltpu.make_async_copy(x_hbm.at[rows], xbuf.at[rows], lsem.at[i])

        for i in range(nch):
            load(i).start()
        g_copy = pltpu.make_async_copy(g_hbm, gbuf, gsem.at[0])
        b_copy = pltpu.make_async_copy(b_hbm, bbuf, gsem.at[1])
        g_copy.start()
        b_copy.start()

        peer = (lax.axis_index("x"), 1 - lax.axis_index("y"))
        barrier = pltpu.get_barrier_semaphore()
        pl.semaphore_signal(barrier, inc=1, device_id=peer,
                            device_id_type=pl.DeviceIdType.MESH)
        sbuf[...] = jnp.zeros(sbuf.shape, jnp.int32)

        def exchange(i):
            return pltpu.make_async_remote_copy(
                src_ref=sbuf.at[i], dst_ref=rbuf.at[i],
                send_sem=ssem, recv_sem=rsem.at[i],
                device_id=peer, device_id_type=pl.DeviceIdType.MESH)

        def diag(rows, shift=0):
            row = lax.broadcasted_iota(jnp.int32, (rows, LANES), 0)
            lane = lax.broadcasted_iota(jnp.int32, (rows, LANES), 1)
            return row + shift == lane

        def pack(col, shift=0):
            return jnp.sum(jnp.where(diag(col.shape[0], shift), col, 0.0),
                           axis=0, keepdims=True)

        def unpack(vec, rows):
            return jnp.sum(jnp.where(diag(rows), vec, 0.0), axis=1, keepdims=True)

        def as_int(v):
            return lax.bitcast_convert_type(v, jnp.int32)

        def as_f32(v):
            return lax.bitcast_convert_type(v, jnp.float32)

        def folded_terms(r0, rows):
            xa = xbuf[pl.ds(r0, rows), 0:LANES]
            xb = xbuf[pl.ds(r0, rows), LANES:2 * LANES]
            return xa + xb, xa * xa + xb * xb

        scale = jnp.full((SUBLANES, LANES), half_inv_n, jnp.float32)

        def mxu_moment(t):
            return lax.dot_general(scale, t, (((1,), (1,)), ((), ())),
                                   preferred_element_type=jnp.float32)[0:1]

        def encode(hm, e2):
            q = hm * hm
            hv = (e2 - q) - q
            floor = jnp.where(e2 <= MAX_SQUARE, q * (2.0 / SAFE_RATIO), jnp.nan)
            low = lax.shift_right_logical(as_int(hm) + 0x8000, 16)
            high = (as_int(hv) + (0x8000 - low)) & HIGH_HALF
            return high | jnp.where(floor <= hv, low, SIGN_BIT)

        for i in range(nch):
            load(i).wait()
            a, rows = MXU_ROWS[i], CHUNKS[i]
            t1, t2 = folded_terms(offs[i] + a, rows - a)
            hm = pack(jnp.sum(t1, axis=1, keepdims=True), a) * half_inv_n
            e2 = pack(jnp.sum(t2, axis=1, keepdims=True), a) * half_inv_n
            sbuf[i, :, a:rows] = encode(hm, e2)[:, a:rows]
            if a > 0:
                t1, t2 = folded_terms(offs[i], a)
                sbuf[i, :, 0:a] = encode(mxu_moment(t1), mxu_moment(t2))
            if i == 0:
                pl.semaphore_wait(barrier, 1)
            exchange(i).start()

        flags = jnp.min(jnp.min(sbuf[...], axis=0))
        for j in range(nblk):
            rows = pl.ds(j * LANES, LANES)
            t1, t2 = folded_terms(j * LANES, LANES)
            hm = jnp.sum(t1, axis=1, keepdims=True) * half_inv_n
            e2 = jnp.sum(t2, axis=1, keepdims=True) * half_inv_n
            hcol[rows, :] = jnp.broadcast_to(hm, (LANES, LANES))
            vcol[rows, :] = jnp.broadcast_to((e2 - 2.0 * hm * hm) + EPS, (LANES, LANES))
        g_copy.wait()
        b_copy.wait()

        def normalize_chunk(i, flags):
            sub = lax.broadcasted_iota(jnp.int32, (SUBLANES, LANES), 0)
            bit0, bit1, bit2 = (sub & 1) != 0, (sub & 2) != 0, (sub & 4) != 0
            g = gbuf[...]
            b = bbuf[...]
            for group in range(CHUNKS[i] // SUBLANES):
                s = [rbuf[i, 0, SUBLANES * group + t] for t in range(SUBLANES)]
                for word in s:
                    flags = flags | word
                pairs = [jnp.where(bit0, s[2 * t + 1], s[2 * t]) for t in range(4)]
                quads = [jnp.where(bit1, pairs[1], pairs[0]),
                         jnp.where(bit1, pairs[3], pairs[2])]
                words = jnp.where(bit2, quads[1], quads[0])
                r = pl.ds(offs[i] + SUBLANES * group, SUBLANES)
                hm_r = as_f32(lax.shift_left(words, 16))
                hm_l = hcol[r, :]
                delta = hm_r - hm_l
                mean = hm_r + hm_l
                var = (vcol[r, :] + as_f32(words)) + delta * delta
                rstd = lax.exp2(jnp.log(var) * (-0.5 / LN2))
                for h in range(n // LANES):
                    c = pl.ds(LANES * h, LANES)
                    gs = g[:, LANES * h:LANES * (h + 1)]
                    bs = b[:, LANES * h:LANES * (h + 1)]
                    o_ref[r, c] = ((xbuf[r, c] - mean) * gs) * rstd + bs
            return flags

        for i in range(nch):
            if i == nch - 1:
                pltpu.make_async_copy(sbuf, sbuf, ssem).wait()
            exchange(i).wait_recv()
            flags = normalize_chunk(i, flags)

        @pl.when(flags < 0)
        def _():
            def centered_stats(j, carry):
                xv = xbuf[pl.ds(pl.multiple_of(j * LANES, LANES), LANES), :]
                mu = jnp.sum(xv, axis=1, keepdims=True) * (1.0 / n)
                d = xv - mu
                m2 = jnp.sum(d * d, axis=1, keepdims=True)
                sfix[j, 0:1, :] = pack(mu * 0.5)
                sfix[j, 1:2, :] = pack(m2 * half_inv_n)
                return carry

            lax.fori_loop(0, nblk, centered_stats, 0)
            fix = pltpu.make_async_remote_copy(
                src_ref=sfix, dst_ref=rfix, send_sem=fsem.at[0], recv_sem=fsem.at[1],
                device_id=peer, device_id_type=pl.DeviceIdType.MESH)
            fix.start()
            fix.wait()

            def renormalize(j, carry):
                rows = pl.ds(pl.multiple_of(j * LANES, LANES), LANES)
                hm_l, hv_l = sfix[j, 0:1, :], sfix[j, 1:2, :]
                hm_r, hv_r = rfix[j, 0:1, :], rfix[j, 1:2, :]
                delta = hm_r - hm_l
                mean = hm_r + hm_l
                rstd = lax.rsqrt((hv_l + hv_r) + (delta * delta + EPS))
                o_ref[rows, :] = ((xbuf[rows, :] - unpack(mean, LANES))
                                  * unpack(rstd, LANES) * gbuf[...] + bbuf[...])
                return carry

            lax.fori_loop(0, nblk, renormalize, 0)

    any_spec = pl.BlockSpec(memory_space=pl.ANY)
    return pl.pallas_call(
        body,
        out_shape=jax.ShapeDtypeStruct((m, n), x.dtype),
        in_specs=[any_spec, any_spec, any_spec],
        out_specs=pl.BlockSpec(memory_space=pltpu.VMEM),
        scratch_shapes=[
            pltpu.VMEM((m, n), jnp.float32),
            pltpu.VMEM((1, n), jnp.float32),
            pltpu.VMEM((1, n), jnp.float32),
            pltpu.VMEM((nblk, 2, LANES), jnp.float32),
            pltpu.VMEM((nblk, 2, LANES), jnp.float32),
            pltpu.VMEM((m, LANES), jnp.float32),
            pltpu.VMEM((m, LANES), jnp.float32),
            pltpu.VMEM((nch, 1, LANES), jnp.int32),
            pltpu.SMEM((nch, 1, LANES), jnp.int32),
            pltpu.SemaphoreType.DMA((nch,)),
            pltpu.SemaphoreType.DMA((2,)),
            pltpu.SemaphoreType.DMA(()),
            pltpu.SemaphoreType.DMA((nch,)),
            pltpu.SemaphoreType.DMA((2,)),
        ],
        compiler_params=pltpu.CompilerParams(
            collective_id=0,
            disable_semaphore_checks=True,
            disable_bounds_checks=True,
        ),
    )(x, gamma.reshape(1, n), beta.reshape(1, n))
```
